```python
import numpy as np

kernel_name = "dist_moe_shared_ep_outshard_n512_d256_e2_h512"

def setup_inputs():
    x = np.random.randn(512, 256).astype(np.float32)
    router_W = np.random.randn(256, 8).astype(np.float32) * 0.1
    scores64 = x.astype(np.float64) @ router_W.astype(np.float64)
    route_idx = np.argsort(-scores64, axis=-1)[:, :1].astype(np.int32)
    expert_W = np.random.randn(8, 256, 512).astype(np.float32) * 0.02
    shared_W = np.random.randn(256, 512).astype(np.float32) * 0.02
    return {"x": x, "router_W": router_W, "route_idx": route_idx, "expert_W": expert_W, "shared_W": shared_W}

def reference(x, router_W, route_idx, expert_W, shared_W):
    scores = x @ router_W
    s_max = scores.max(axis=-1, keepdims=True)
    probs = np.exp(scores - s_max)
    probs = probs / probs.sum(axis=-1, keepdims=True)
    shared = x @ shared_W
    out = np.zeros((512, 512), dtype=np.float32)
    for i in range(512):
        e = int(route_idx[i, 0])
        out[i] = shared[i] + probs[i, e] * (x[i] @ expert_W[e])
    return out
```

```python
import contextlib
import jax
import jax.numpy as jnp
from jax import lax
from jax.experimental import pallas as pl
from jax.experimental.pallas import tpu as pltpu

N_DEV = 4
N_TOK = 512
D = 256
H = 512
N_EXP = 8
BLK = N_TOK // N_DEV
CH = 16
MAXCH = BLK // CH
NSLOT = 12
RROWS = NSLOT * CH
NB = 4
CB = H // NB
SEND_ORDER = (2, 1, 3)


def scope(n):
    del n
    return contextlib.nullcontext()


def pallas_dist_moe_shared_ep_outshard_n512_d256_e2_h512_kernel(x, router_W, route_idx, expert_W, shared_W):
    bf16 = jnp.bfloat16
    f32 = jnp.float32
    i32 = jnp.int32

    def body(x_hbm, rwt_hbm, r_hbm, ew_hbm, sw_hbm, out_ref,
             xv, rv, wv, wb, swv, rwv, xc_ref, ybuf, rbuf, pos_ref, cnt_s,
             ld_sems, send_sems, recv_sems):
        my = lax.axis_index("i")

        rbuf[...] = jnp.zeros_like(rbuf)
        barrier_sem = pltpu.get_barrier_semaphore()
        for k in range(1, N_DEV):
            pl.semaphore_signal(barrier_sem, inc=1, device_id=((my + k) % N_DEV,),
                                device_id_type=pl.DeviceIdType.MESH)

        dsts = [(my - kk) % N_DEV for kk in SEND_ORDER] + [my]

        def x_copy(idx):
            rows = pl.ds(pl.multiple_of(dsts[idx] * BLK, BLK), BLK)
            return pltpu.make_async_copy(x_hbm.at[rows], xv.at[rows], ld_sems.at[1 + idx])

        def w_copy(j):
            cols = pl.ds(j * CB, CB)
            return pltpu.make_async_copy(ew_hbm.at[:, :, cols], wv.at[:, :, cols], ld_sems.at[5 + j])

        r_cp = pltpu.make_async_copy(r_hbm, rv, ld_sems.at[0])
        sw_cp = pltpu.make_async_copy(sw_hbm, swv, ld_sems.at[5 + NB])
        rw_cp = pltpu.make_async_copy(rwt_hbm, rwv, ld_sems.at[6 + NB])
        r_cp.start()
        for idx in range(N_DEV - 1):
            x_copy(idx).start()
        for j in range(NB):
            w_copy(j).start()
        x_copy(N_DEV - 1).start()
        sw_cp.start()
        rw_cp.start()

        sub = lax.broadcasted_iota(i32, (BLK, BLK), 0)
        lane = lax.broadcasted_iota(i32, (BLK, BLK), 1)
        tri = jnp.where(sub < lane, 1.0, 0.0).astype(bf16)

        with scope("s_book"):
            r_cp.wait()
            r4 = rv[...]
            chip4 = r4 >> 1
            c16 = jnp.concatenate([chip4] * N_DEV, axis=0)
            srow = lax.broadcasted_iota(i32, (N_DEV * N_DEV, BLK), 0) >> 2
            m16 = c16 == srow
            pos16 = jnp.dot(jnp.where(m16, 1.0, 0.0).astype(bf16), tri, preferred_element_type=f32)
            pos_ref[...] = pos16.astype(i32)
            cnt_col = jnp.sum(jnp.where(m16, 1, 0).astype(i32), axis=1, keepdims=True)
            for i in range(N_DEV * N_DEV):
                cnt_s[i] = cnt_col[i, 0]

        def nch(s, d):
            return (cnt_s[N_DEV * s + d] + (CH - 1)) // CH

        def off_ch(s, d):
            kk = (s - d) % N_DEV
            kk = jnp.where(kk == 0, N_DEV, kk)
            o = jnp.int32(0)
            for k2 in range(1, N_DEV):
                o = o + jnp.where(k2 < kk, nch((d + k2) % N_DEV, d), 0)
            return o

        def compact(idx):
            d = dsts[idx]
            rrow = rv[pl.ds(d, 1), :]
            prow = pos_ref[pl.ds(N_DEV * my + d, 1), :]
            eqpos = jnp.broadcast_to(prow, (BLK, BLK)) == sub
            rb = jnp.broadcast_to(rrow, (BLK, BLK))
            p0 = jnp.where(eqpos & (rb == 2 * my), 1.0, 0.0).astype(bf16)
            p1 = jnp.where(eqpos & (rb == 2 * my + 1), 1.0, 0.0).astype(bf16)
            xd = xv[pl.ds(pl.multiple_of(d * BLK, BLK), BLK), :].astype(bf16)
            xc_ref[idx, :, 0:D] = jnp.dot(p0, xd, preferred_element_type=f32).astype(bf16)
            xc_ref[idx, :, D:2 * D] = jnp.dot(p1, xd, preferred_element_type=f32).astype(bf16)

        with scope("s_compact"):
            for idx in range(N_DEV - 1):
                x_copy(idx).wait()
                compact(idx)

        n_send = [nch(my, dsts[idx]) for idx in range(N_DEV - 1)]
        o_send = [off_ch(my, dsts[idx]) for idx in range(N_DEV - 1)]

        def send_desc(idx, j):
            rows = n_send[idx] * CH
            return pltpu.make_async_remote_copy(
                src_ref=ybuf.at[idx, pl.ds(0, rows), pl.ds(j * CB, CB)],
                dst_ref=rbuf.at[pl.ds(pl.multiple_of(o_send[idx] * CH, CH), rows), pl.ds(j * CB, CB)],
                send_sem=send_sems.at[j * (N_DEV - 1) + idx],
                recv_sem=recv_sems.at[j * (N_DEV - 1) + SEND_ORDER[idx] - 1],
                device_id=(dsts[idx],), device_id_type=pl.DeviceIdType.MESH)

        with scope("s_barwait"):
            pl.semaphore_wait(barrier_sem, N_DEV - 1)

        for j in range(NB):
            with scope(f"s_chunk{j}"):
                cols = pl.ds(j * CB, CB)
                w_copy(j).wait()
                wb[0:D, cols] = wv[0, :, cols].astype(bf16)
                wb[D:2 * D, cols] = wv[1, :, cols].astype(bf16)
                wj = wb[:, cols]
                for idx in range(N_DEV - 1):
                    ybuf[idx, :, cols] = jnp.dot(xc_ref[idx], wj, preferred_element_type=f32).astype(bf16)
                for idx in range(N_DEV - 1):
                    @pl.when(n_send[idx] > 0)
                    def _(idx=idx, j=j):
                        send_desc(idx, j).start()

        with scope("s_own"):
            x_copy(N_DEV - 1).wait()
            compact(N_DEV - 1)
            y_own = jnp.dot(xc_ref[N_DEV - 1], wb[...], preferred_element_type=f32).astype(bf16)
            o_own = off_ch(my, my)
            n_own = nch(my, my)
            for c in range(MAXCH):
                @pl.when(c < n_own)
                def _(c=c):
                    rbuf[pl.ds(pl.multiple_of((o_own + c) * CH, CH), CH), :] = y_own[c * CH:(c + 1) * CH, :]

        with scope("s_gate"):
            rrow = rv[pl.ds(my, 1), :]
            crow = rrow >> 1
            g_row = jnp.zeros((1, BLK), i32)
            for s in range(N_DEV):
                ps = pos_ref[pl.ds(N_DEV * s + my, 1), :]
                g_row = jnp.where(crow == s, ps + off_ch(s, my) * CH, g_row)
            x_own = xv[pl.ds(pl.multiple_of(my * BLK, BLK), BLK), :]
            rw_cp.wait()
            scores_t = lax.dot_general(rwv[...], x_own, (((1,), (1,)), ((), ())),
                                       preferred_element_type=f32, precision=lax.Precision.HIGHEST)
            s_max = jnp.max(scores_t, axis=0, keepdims=True)
            ex = jnp.exp(scores_t - s_max)
            probs_t = ex / jnp.sum(ex, axis=0, keepdims=True)
            e_iota = lax.broadcasted_iota(i32, (N_EXP, BLK), 0)
            p_row = jnp.sum(jnp.where(e_iota == jnp.broadcast_to(rrow, (N_EXP, BLK)), probs_t, 0.0),
                            axis=0, keepdims=True)
            g_iota = lax.broadcasted_iota(i32, (RROWS, BLK), 0)
            pg = jnp.where(g_iota == jnp.broadcast_to(g_row, (RROWS, BLK)),
                           jnp.broadcast_to(p_row, (RROWS, BLK)), 0.0)
            pgt = pg.T.astype(bf16)
            sw_cp.wait()
            shared = jnp.dot(x_own.astype(bf16), swv[...].astype(bf16), preferred_element_type=f32)

        n_recv = [nch((my + k) % N_DEV, my) for k in range(1, N_DEV)]
        o_recv = [off_ch((my + k) % N_DEV, my) for k in range(1, N_DEV)]
        for j in range(NB):
            with scope(f"s_fin{j}"):
                cols = pl.ds(j * CB, CB)
                for k in range(1, N_DEV):
                    @pl.when(n_recv[k - 1] > 0)
                    def _(k=k, j=j):
                        rows = n_recv[k - 1] * CH
                        pltpu.make_async_remote_copy(
                            src_ref=ybuf.at[0, pl.ds(0, rows), pl.ds(j * CB, CB)],
                            dst_ref=rbuf.at[pl.ds(pl.multiple_of(o_recv[k - 1] * CH, CH), rows), pl.ds(j * CB, CB)],
                            send_sem=send_sems.at[0],
                            recv_sem=recv_sems.at[j * (N_DEV - 1) + k - 1],
                            device_id=(my,), device_id_type=pl.DeviceIdType.MESH).wait_recv()
                acc = jnp.dot(pgt, rbuf[:, cols], preferred_element_type=f32)
                out_ref[:, cols] = shared[:, j * CB:(j + 1) * CB] + acc

        with scope("s_waitsend"):
            for j in range(NB):
                for idx in range(N_DEV - 1):
                    @pl.when(n_send[idx] > 0)
                    def _(idx=idx, j=j):
                        send_desc(idx, j).wait_send()

    return pl.pallas_call(
        body,
        out_shape=jax.ShapeDtypeStruct((BLK, H), jnp.float32),
        in_specs=[pl.BlockSpec(memory_space=pl.ANY)] * 5,
        out_specs=pl.BlockSpec(memory_space=pltpu.VMEM),
        scratch_shapes=[
            pltpu.VMEM((N_TOK, D), f32),
            pltpu.VMEM((N_DEV, BLK), i32),
            pltpu.VMEM((2, D, H), f32),
            pltpu.VMEM((2 * D, H), bf16),
            pltpu.VMEM((D, H), f32),
            pltpu.VMEM((N_EXP, D), f32),
            pltpu.VMEM((N_DEV, BLK, 2 * D), bf16),
            pltpu.VMEM((N_DEV - 1, BLK, H), bf16),
            pltpu.VMEM((RROWS, H), bf16),
            pltpu.VMEM((N_DEV * N_DEV, BLK), i32),
            pltpu.SMEM((N_DEV * N_DEV,), i32),
            pltpu.SemaphoreType.DMA((7 + NB,)),
            pltpu.SemaphoreType.DMA(((N_DEV - 1) * NB,)),
            pltpu.SemaphoreType.DMA(((N_DEV - 1) * NB,)),
        ],
        compiler_params=pltpu.CompilerParams(collective_id=0),
    )(x, router_W.T, route_idx.reshape(N_DEV, BLK), expert_W, shared_W)
```

```python
import jax
import jax.numpy as jnp
from jax import lax
from jax.experimental import pallas as pl
from jax.experimental.pallas import tpu as pltpu

N_DEV = 4
N_TOK = 512
D = 256
H = 512
N_EXP = 8
BLK = N_TOK // N_DEV
CH = 16
NSLOT = 12
RROWS = NSLOT * CH
NB = 4
CB = H // NB
TM = 64
NT = BLK // TM
SEND_ORDER = (2, 1, 3)
N_LD = 7 + NB


def pallas_dist_moe_shared_ep_outshard_n512_d256_e2_h512_kernel(
    x: jax.Array,
    router_W: jax.Array,
    route_idx: jax.Array,
    expert_W: jax.Array,
    shared_W: jax.Array,
):
    bf16 = jnp.bfloat16
    f32 = jnp.float32
    i32 = jnp.int32

    def body(x_hbm, rwt_hbm, r_hbm, ew_hbm, sw_hbm, out_ref,
             xv, rv, wv, wb, swv, rwv, xc_ref, ybuf, rbuf, pos_ref, cnt_s,
             ld_sems, send_sems, recv_sems):
        my = lax.axis_index("i")

        rbuf[...] = jnp.zeros_like(rbuf)
        barrier_sem = pltpu.get_barrier_semaphore()
        for k in range(1, N_DEV):
            pl.semaphore_signal(barrier_sem, inc=1, device_id=((my + k) % N_DEV,),
                                device_id_type=pl.DeviceIdType.MESH)

        dsts = [(my - kk) % N_DEV for kk in SEND_ORDER] + [my]

        def x_copy(idx):
            rows = pl.ds(pl.multiple_of(dsts[idx] * BLK, BLK), BLK)
            return pltpu.make_async_copy(x_hbm.at[rows], xv.at[rows], ld_sems.at[1 + idx])

        def w_copy(j):
            cols = pl.ds(j * CB, CB)
            return pltpu.make_async_copy(ew_hbm.at[:, :, cols], wv.at[:, :, cols], ld_sems.at[5 + j])

        r_cp = pltpu.make_async_copy(r_hbm, rv, ld_sems.at[0])
        sw_cp = pltpu.make_async_copy(sw_hbm, swv, ld_sems.at[5 + NB])
        rw_cp = pltpu.make_async_copy(rwt_hbm, rwv, ld_sems.at[6 + NB])
        r_cp.start()
        for idx in range(N_DEV - 1):
            x_copy(idx).start()
        for j in range(NB):
            w_copy(j).start()
        x_copy(N_DEV - 1).start()
        sw_cp.start()
        rw_cp.start()

        sub = lax.broadcasted_iota(i32, (BLK, BLK), 0)
        lane = lax.broadcasted_iota(i32, (BLK, BLK), 1)
        tri = jnp.where(sub < lane, 1.0, 0.0).astype(bf16)

        r_cp.wait()
        r4 = rv[...]
        chip4 = r4 >> 1
        c16 = jnp.concatenate([chip4] * N_DEV, axis=0)
        srow = lax.broadcasted_iota(i32, (N_DEV * N_DEV, BLK), 0) >> 2
        m16 = c16 == srow
        pos16 = jnp.dot(jnp.where(m16, 1.0, 0.0).astype(bf16), tri, preferred_element_type=f32)
        pos_ref[...] = pos16.astype(i32)
        cnt_col = jnp.sum(jnp.where(m16, 1, 0).astype(i32), axis=1, keepdims=True)
        for i in range(N_DEV * N_DEV):
            cnt_s[i] = cnt_col[i, 0]

        def nch(s, d):
            return (cnt_s[N_DEV * s + d] + (CH - 1)) // CH

        def off_ch(s, d):
            kk = (s - d) % N_DEV
            kk = jnp.where(kk == 0, N_DEV, kk)
            o = jnp.int32(0)
            for k2 in range(1, N_DEV):
                o = o + jnp.where(k2 < kk, nch((d + k2) % N_DEV, d), 0)
            return o

        def compact(idx, t):
            d = dsts[idx]
            rrow = rv[pl.ds(d, 1), :]
            prow = pos_ref[pl.ds(N_DEV * my + d, 1), :]
            subt = sub[0:TM, :] + t * TM
            eqpos = jnp.broadcast_to(prow, (TM, BLK)) == subt
            rb = jnp.broadcast_to(rrow, (TM, BLK))
            p0 = jnp.where(eqpos & (rb == 2 * my), 1.0, 0.0).astype(bf16)
            p1 = jnp.where(eqpos & (rb == 2 * my + 1), 1.0, 0.0).astype(bf16)
            xd = xv[pl.ds(pl.multiple_of(d * BLK, BLK), BLK), :].astype(bf16)
            rows = pl.ds(t * TM, TM)
            xc_ref[idx, rows, 0:D] = jnp.dot(p0, xd, preferred_element_type=f32).astype(bf16)
            xc_ref[idx, rows, D:2 * D] = jnp.dot(p1, xd, preferred_element_type=f32).astype(bf16)

        big = jnp.bool_(False)
        for idx in range(N_DEV):
            big = jnp.logical_or(big, cnt_s[N_DEV * my + dsts[idx]] > TM)

        for idx in range(N_DEV - 1):
            x_copy(idx).wait()
            compact(idx, 0)
        for t in range(1, NT):
            @pl.when(big)
            def _(t=t):
                for idx in range(N_DEV - 1):
                    compact(idx, t)

        n_send = [nch(my, dsts[idx]) for idx in range(N_DEV - 1)]
        o_send = [off_ch(my, dsts[idx]) for idx in range(N_DEV - 1)]

        def send_desc(idx, j):
            rows = n_send[idx] * CH
            return pltpu.make_async_remote_copy(
                src_ref=ybuf.at[idx, pl.ds(0, rows), pl.ds(j * CB, CB)],
                dst_ref=rbuf.at[pl.ds(pl.multiple_of(o_send[idx] * CH, CH), rows), pl.ds(j * CB, CB)],
                send_sem=send_sems.at[0],
                recv_sem=recv_sems.at[j * (N_DEV - 1) + SEND_ORDER[idx] - 1],
                device_id=(dsts[idx],), device_id_type=pl.DeviceIdType.MESH)

        pl.semaphore_wait(barrier_sem, N_DEV - 1)

        for j in range(NB):
            cols = pl.ds(j * CB, CB)
            w_copy(j).wait()
            wb[0:D, cols] = wv[0, :, cols].astype(bf16)
            wb[D:2 * D, cols] = wv[1, :, cols].astype(bf16)
            wj = wb[:, cols]
            for idx in range(N_DEV - 1):
                ybuf[idx, 0:TM, cols] = jnp.dot(xc_ref[idx, 0:TM, :], wj,
                                                preferred_element_type=f32).astype(bf16)
            for t in range(1, NT):
                @pl.when(big)
                def _(t=t, cols=cols, wj=wj):
                    for idx in range(N_DEV - 1):
                        ybuf[idx, pl.ds(t * TM, TM), cols] = jnp.dot(
                            xc_ref[idx, pl.ds(t * TM, TM), :], wj,
                            preferred_element_type=f32).astype(bf16)
            for idx in range(N_DEV - 1):
                @pl.when(n_send[idx] > 0)
                def _(idx=idx, j=j):
                    send_desc(idx, j).start()

        x_copy(N_DEV - 1).wait()
        compact(N_DEV - 1, 0)
        o_own = off_ch(my, my)
        n_own = nch(my, my)
        y_own0 = jnp.dot(xc_ref[N_DEV - 1, 0:TM, :], wb[...], preferred_element_type=f32).astype(bf16)
        for c in range(TM // CH):
            @pl.when(c < n_own)
            def _(c=c):
                rbuf[pl.ds(pl.multiple_of((o_own + c) * CH, CH), CH), :] = y_own0[c * CH:(c + 1) * CH, :]
        for t in range(1, NT):
            @pl.when(big)
            def _(t=t):
                compact(N_DEV - 1, t)
                y_own = jnp.dot(xc_ref[N_DEV - 1, pl.ds(t * TM, TM), :], wb[...],
                                preferred_element_type=f32).astype(bf16)
                for c in range(TM // CH):
                    cc = t * (TM // CH) + c

                    @pl.when(cc < n_own)
                    def _(cc=cc, c=c):
                        rbuf[pl.ds(pl.multiple_of((o_own + cc) * CH, CH), CH), :] = \
                            y_own[c * CH:(c + 1) * CH, :]

        rrow = rv[pl.ds(my, 1), :]
        crow = rrow >> 1
        g_row = jnp.zeros((1, BLK), i32)
        for s in range(N_DEV):
            ps = pos_ref[pl.ds(N_DEV * s + my, 1), :]
            g_row = jnp.where(crow == s, ps + off_ch(s, my) * CH, g_row)
        x_own = xv[pl.ds(pl.multiple_of(my * BLK, BLK), BLK), :]
        rw_cp.wait()
        scores_t = lax.dot_general(rwv[...], x_own, (((1,), (1,)), ((), ())),
                                   preferred_element_type=f32, precision=lax.Precision.HIGHEST)
        s_max = jnp.max(scores_t, axis=0, keepdims=True)
        ex = jnp.exp(scores_t - s_max)
        probs_t = ex / jnp.sum(ex, axis=0, keepdims=True)
        e_iota = lax.broadcasted_iota(i32, (N_EXP, BLK), 0)
        p_row = jnp.sum(jnp.where(e_iota == jnp.broadcast_to(rrow, (N_EXP, BLK)), probs_t, 0.0),
                        axis=0, keepdims=True)
        g_iota = lax.broadcasted_iota(i32, (RROWS, BLK), 0)
        pg = jnp.where(g_iota == jnp.broadcast_to(g_row, (RROWS, BLK)),
                       jnp.broadcast_to(p_row, (RROWS, BLK)), 0.0)
        pgt = pg.T.astype(bf16)
        sw_cp.wait()
        shared = jnp.dot(x_own.astype(bf16), swv[...].astype(bf16), preferred_element_type=f32)

        n_recv = [nch((my + k) % N_DEV, my) for k in range(1, N_DEV)]
        o_recv = [off_ch((my + k) % N_DEV, my) for k in range(1, N_DEV)]
        for j in range(NB):
            cols = pl.ds(j * CB, CB)
            for k in range(1, N_DEV):
                @pl.when(n_recv[k - 1] > 0)
                def _(k=k, j=j):
                    rows = n_recv[k - 1] * CH
                    pltpu.make_async_remote_copy(
                        src_ref=ybuf.at[0, pl.ds(0, rows), pl.ds(j * CB, CB)],
                        dst_ref=rbuf.at[pl.ds(pl.multiple_of(o_recv[k - 1] * CH, CH), rows),
                                        pl.ds(j * CB, CB)],
                        send_sem=send_sems.at[0],
                        recv_sem=recv_sems.at[j * (N_DEV - 1) + k - 1],
                        device_id=(my,), device_id_type=pl.DeviceIdType.MESH).wait_recv()
            acc = jnp.dot(pgt, rbuf[:, cols], preferred_element_type=f32)
            out_ref[:, cols] = shared[:, j * CB:(j + 1) * CB] + acc

        for j in range(NB):
            for idx in range(N_DEV - 1):
                @pl.when(n_send[idx] > 0)
                def _(idx=idx, j=j):
                    send_desc(idx, j).wait_send()

    return pl.pallas_call(
        body,
        out_shape=jax.ShapeDtypeStruct((BLK, H), jnp.float32),
        in_specs=[pl.BlockSpec(memory_space=pl.ANY)] * 5,
        out_specs=pl.BlockSpec(memory_space=pltpu.VMEM),
        scratch_shapes=[
            pltpu.VMEM((N_TOK, D), f32),
            pltpu.VMEM((N_DEV, BLK), i32),
            pltpu.VMEM((2, D, H), f32),
            pltpu.VMEM((2 * D, H), bf16),
            pltpu.VMEM((D, H), f32),
            pltpu.VMEM((N_EXP, D), f32),
            pltpu.VMEM((N_DEV, BLK, 2 * D), bf16),
            pltpu.VMEM((N_DEV - 1, BLK, H), bf16),
            pltpu.VMEM((RROWS, H), bf16),
            pltpu.VMEM((N_DEV * N_DEV, BLK), i32),
            pltpu.SMEM((N_DEV * N_DEV,), i32),
            pltpu.SemaphoreType.DMA((N_LD,)),
            pltpu.SemaphoreType.DMA((1,)),
            pltpu.SemaphoreType.DMA(((N_DEV - 1) * NB,)),
        ],
        compiler_params=pltpu.CompilerParams(collective_id=0),
    )(x, router_W.T, route_idx.reshape(N_DEV, BLK), expert_W, shared_W)
```
